```python
import numpy as np

kernel_name = "dist_mean_ax0_xy_m1024_n512"

def setup_inputs():
    return {"x": np.random.randn(2048, 1024).astype(np.float32)}

def reference(x: np.ndarray) -> np.ndarray:
    return np.mean(x, axis=0, keepdims=True)
```

```python
import jax
import jax.numpy as jnp
from jax import lax
from jax.experimental import pallas as pl
from jax.experimental.pallas import tpu as pltpu

_ROW_CHUNKS = (768, 192)
_LAST_ROWS = 64
_TAIL_COLS = 128
_ACC_ROWS = 16


def pallas_dist_mean_ax0_xy_m1024_n512_kernel(
    x: jax.Array,
):
    m, n = x.shape
    assert sum(_ROW_CHUNKS) + _LAST_ROWS == m
    n_full = len(_ROW_CHUNKS)
    starts = [sum(_ROW_CHUNKS[:i]) for i in range(n_full)]
    last0 = m - _LAST_ROWS
    pieces = ((0, n - _TAIL_COLS), (n - _TAIL_COLS, _TAIL_COLS))
    mesh_id = pl.DeviceIdType.MESH

    def kernel_body(x_hbm, out_ref, xbuf, sbuf, rbuf, load_sems, send_sem, recv_sem):
        scale = 1.0 / (m * lax.axis_size("x"))
        neighbour = (1 - lax.axis_index("x"), lax.axis_index("y"))
        barrier = pltpu.get_barrier_semaphore()

        def load(rows, cols, i):
            copy = pltpu.make_async_copy(
                x_hbm.at[rows, cols], xbuf.at[rows, cols], load_sems.at[i]
            )
            copy.start()
            return copy

        def exchange(src, dst):
            return pltpu.make_async_remote_copy(
                src, dst, send_sem, recv_sem,
                device_id=neighbour, device_id_type=mesh_id,
            )

        def row_sum(rows, cols):
            v = xbuf[rows, cols]
            return v.reshape(-1, _ACC_ROWS, v.shape[1]).sum(axis=0)

        all_cols = pl.ds(0, n)
        full = [
            load(pl.ds(starts[i], _ROW_CHUNKS[i]), all_cols, i) for i in range(n_full)
        ]
        last_rows = pl.ds(last0, _LAST_ROWS)
        tail = [
            load(last_rows, pl.ds(c0, w), n_full + j)
            for j, (c0, w) in enumerate(pieces)
        ]
        pl.semaphore_signal(barrier, inc=1, device_id=neighbour, device_id_type=mesh_id)

        acc = None
        for i in range(n_full):
            if i == n_full - 1:
                pl.semaphore_wait(barrier, 1)
            full[i].wait()
            part = row_sum(pl.ds(starts[i], _ROW_CHUNKS[i]), all_cols)
            acc = part if acc is None else acc + part

        for j, (c0, w) in enumerate(pieces):
            cols = pl.ds(c0, w)
            tail[j].wait()
            part = acc[:, c0:c0 + w] + row_sum(last_rows, cols)
            part = part.reshape(-1, 8, w).sum(axis=0)
            sbuf[:, cols] = jnp.sum(part, axis=0, keepdims=True) * scale
            exchange(sbuf.at[:, cols], rbuf.at[:, cols]).start()

        both = exchange(sbuf, rbuf)
        both.wait_recv()
        out_ref[...] = sbuf[...] + rbuf[...]
        both.wait_send()

    return pl.pallas_call(
        kernel_body,
        out_shape=jax.ShapeDtypeStruct((1, n), x.dtype),
        in_specs=[pl.BlockSpec(memory_space=pltpu.HBM)],
        out_specs=pl.BlockSpec(memory_space=pltpu.VMEM),
        scratch_shapes=[
            pltpu.VMEM((m, n), x.dtype),
            pltpu.VMEM((1, n), x.dtype),
            pltpu.VMEM((1, n), x.dtype),
            pltpu.SemaphoreType.DMA((n_full + len(pieces),)),
            pltpu.SemaphoreType.DMA,
            pltpu.SemaphoreType.DMA,
        ],
        compiler_params=pltpu.CompilerParams(
            collective_id=0, disable_semaphore_checks=True
        ),
    )(x)
```

```python
import jax
import jax.numpy as jnp
from jax import lax
from jax.experimental import pallas as pl
from jax.experimental.pallas import tpu as pltpu

_ROW_CHUNKS = (768, 192)
_LAST_ROWS = 64
_TAIL_COLS = 128
_ACC_ROWS = 16


def _tree_sum(vs):
    while len(vs) > 1:
        vs = [
            vs[i] + vs[i + 1] if i + 1 < len(vs) else vs[i]
            for i in range(0, len(vs), 2)
        ]
    return vs[0]


def pallas_dist_mean_ax0_xy_m1024_n512_kernel(
    x: jax.Array,
):
    m, n = x.shape
    assert sum(_ROW_CHUNKS) + _LAST_ROWS == m
    n_full = len(_ROW_CHUNKS)
    starts = [sum(_ROW_CHUNKS[:i]) for i in range(n_full)]
    last0 = m - _LAST_ROWS
    pieces = ((0, n - _TAIL_COLS), (n - _TAIL_COLS, _TAIL_COLS))
    mesh_id = pl.DeviceIdType.MESH

    def kernel_body(
        x_hbm, out_ref, xbuf, wide_buf, tail_buf, sbuf, rbuf,
        load_sems, send_sem, recv_sem,
    ):
        scale = 1.0 / (m * lax.axis_size("x"))
        neighbour = (1 - lax.axis_index("x"), lax.axis_index("y"))
        barrier = pltpu.get_barrier_semaphore()
        piece_bufs = (wide_buf, tail_buf)

        def load(src, dst, i):
            copy = pltpu.make_async_copy(src, dst, load_sems.at[i])
            copy.start()
            return copy

        def exchange(src, dst):
            return pltpu.make_async_remote_copy(
                src, dst, send_sem, recv_sem,
                device_id=neighbour, device_id_type=mesh_id,
            )

        chunks = [pl.ds(starts[i], _ROW_CHUNKS[i]) for i in range(n_full)]
        full = [
            load(x_hbm.at[chunks[i]], xbuf.at[chunks[i]], i) for i in range(n_full)
        ]
        last = [
            load(
                x_hbm.at[pl.ds(last0, _LAST_ROWS), pl.ds(c0, w)],
                piece_bufs[j],
                n_full + j,
            )
            for j, (c0, w) in enumerate(pieces)
        ]
        pl.semaphore_signal(barrier, inc=1, device_id=neighbour, device_id_type=mesh_id)

        acc = None
        for i in range(n_full):
            if i == n_full - 1:
                pl.semaphore_wait(barrier, 1)
            full[i].wait()
            v = xbuf[chunks[i], :]
            part = v.reshape(-1, _ACC_ROWS, n).sum(axis=0)
            acc = part if acc is None else acc + part
        acc = acc.reshape(-1, 8, n).sum(axis=0)

        for j, (c0, w) in enumerate(pieces):
            buf = piece_bufs[j]
            last[j].wait()
            part = _tree_sum([buf[pl.ds(r, 8), :] for r in range(0, _LAST_ROWS, 8)])
            part = part + acc[:, c0:c0 + w]
            cols = pl.ds(c0, w)
            sbuf[:, cols] = jnp.sum(part, axis=0, keepdims=True) * scale
            exchange(sbuf.at[:, cols], rbuf.at[:, cols]).start()

        both = exchange(sbuf, rbuf)
        mine = sbuf[...]
        both.wait_send()
        both.wait_recv()
        out_ref[...] = mine + rbuf[...]

    return pl.pallas_call(
        kernel_body,
        out_shape=jax.ShapeDtypeStruct((1, n), x.dtype),
        in_specs=[pl.BlockSpec(memory_space=pltpu.HBM)],
        out_specs=pl.BlockSpec(memory_space=pltpu.VMEM),
        scratch_shapes=[
            pltpu.VMEM((last0, n), x.dtype),
            pltpu.VMEM((_LAST_ROWS, pieces[0][1]), x.dtype),
            pltpu.VMEM((_LAST_ROWS, pieces[1][1]), x.dtype),
            pltpu.VMEM((1, n), x.dtype),
            pltpu.VMEM((1, n), x.dtype),
            pltpu.SemaphoreType.DMA((n_full + len(pieces),)),
            pltpu.SemaphoreType.DMA,
            pltpu.SemaphoreType.DMA,
        ],
        compiler_params=pltpu.CompilerParams(
            collective_id=0, disable_semaphore_checks=True
        ),
    )(x)
```

```python
import jax
import jax.numpy as jnp
from jax import lax
from jax.experimental import pallas as pl
from jax.experimental.pallas import tpu as pltpu

_ROW_CHUNKS = (768, 192)
_LAST_ROWS = 64
_TAIL_COLS = 128
_ACC_ROWS = 16


def _tree_sum(vs):
    while len(vs) > 1:
        vs = [
            vs[i] + vs[i + 1] if i + 1 < len(vs) else vs[i]
            for i in range(0, len(vs), 2)
        ]
    return vs[0]


def pallas_dist_mean_ax0_xy_m1024_n512_kernel(
    x: jax.Array,
):
    m, n = x.shape
    assert sum(_ROW_CHUNKS) + _LAST_ROWS == m
    n_full = len(_ROW_CHUNKS)
    starts = [sum(_ROW_CHUNKS[:i]) for i in range(n_full)]
    last0 = m - _LAST_ROWS
    pieces = ((0, n - _TAIL_COLS), (n - _TAIL_COLS, _TAIL_COLS))
    mesh_id = pl.DeviceIdType.MESH

    def kernel_body(
        x_hbm, out_ref, xbuf, wide_buf, tail_buf, sbuf, rbuf,
        load_sems, send_sems, recv_sems,
    ):
        scale = 1.0 / (m * lax.axis_size("x"))
        neighbour = (1 - lax.axis_index("x"), lax.axis_index("y"))
        barrier = pltpu.get_barrier_semaphore()
        piece_bufs = (wide_buf, tail_buf)

        def load(src, dst, i):
            copy = pltpu.make_async_copy(src, dst, load_sems.at[i])
            copy.start()
            return copy

        chunks = [pl.ds(starts[i], _ROW_CHUNKS[i]) for i in range(n_full)]
        full = [
            load(x_hbm.at[chunks[i]], xbuf.at[chunks[i]], i) for i in range(n_full)
        ]
        last = [
            load(
                x_hbm.at[pl.ds(last0, _LAST_ROWS), pl.ds(c0, w)],
                piece_bufs[j],
                n_full + j,
            )
            for j, (c0, w) in enumerate(pieces)
        ]
        pl.semaphore_signal(barrier, inc=1, device_id=neighbour, device_id_type=mesh_id)

        acc = None
        for i in range(n_full):
            if i == n_full - 1:
                pl.semaphore_wait(barrier, 1)
            full[i].wait()
            v = xbuf[chunks[i], :]
            part = v.reshape(-1, _ACC_ROWS, n).sum(axis=0)
            acc = part if acc is None else acc + part
        acc = acc.reshape(-1, 8, n).sum(axis=0)

        swaps = []
        for j, (c0, w) in enumerate(pieces):
            buf = piece_bufs[j]
            last[j].wait()
            part = _tree_sum([buf[pl.ds(r, 8), :] for r in range(0, _LAST_ROWS, 8)])
            part = part + acc[:, c0:c0 + w]
            cols = pl.ds(c0, w)
            sbuf[:, cols] = jnp.sum(part, axis=0, keepdims=True) * scale
            swap = pltpu.make_async_remote_copy(
                sbuf.at[:, cols], rbuf.at[:, cols], send_sems.at[j], recv_sems.at[j],
                device_id=neighbour, device_id_type=mesh_id,
            )
            swap.start()
            swaps.append(swap)

        for swap in swaps:
            swap.wait_send()
        mine = sbuf[...]
        for swap in swaps:
            swap.wait_recv()
        out_ref[...] = mine + rbuf[...]

    return pl.pallas_call(
        kernel_body,
        out_shape=jax.ShapeDtypeStruct((1, n), x.dtype),
        in_specs=[pl.BlockSpec(memory_space=pltpu.HBM)],
        out_specs=pl.BlockSpec(memory_space=pltpu.VMEM),
        scratch_shapes=[
            pltpu.VMEM((last0, n), x.dtype),
            pltpu.VMEM((_LAST_ROWS, pieces[0][1]), x.dtype),
            pltpu.VMEM((_LAST_ROWS, pieces[1][1]), x.dtype),
            pltpu.VMEM((1, n), x.dtype),
            pltpu.VMEM((1, n), x.dtype),
            pltpu.SemaphoreType.DMA((n_full + len(pieces),)),
            pltpu.SemaphoreType.DMA((len(pieces),)),
            pltpu.SemaphoreType.DMA((len(pieces),)),
        ],
        compiler_params=pltpu.CompilerParams(
            collective_id=0, disable_semaphore_checks=True
        ),
    )(x)
```
